```python
import numpy as np

kernel_name = "dist_ar_xy_y_m256_n256"

def setup_inputs():
    return {"x": np.random.randn(512, 256).astype(np.float32)}

def reference(x: np.ndarray) -> np.ndarray:
    return x.reshape(2, 256, 256).sum(axis=0)
```

```python
import jax
import jax.numpy as jnp
from jax import lax
from jax.experimental import pallas as pl
from jax.experimental.pallas import tpu as pltpu


def pallas_dist_ar_xy_y_m256_n256_kernel(
x: jax.Array,
):
    def kernel_body(x_ref, o_ref, send_buf, recv_buf, send_sem, recv_sem):
        my_x = lax.axis_index("x")
        my_y = lax.axis_index("y")
        peer = (my_x, 1 - my_y)

        barrier = pltpu.get_barrier_semaphore()
        pl.semaphore_signal(
            barrier, inc=1, device_id=peer, device_id_type=pl.DeviceIdType.MESH
        )
        send_buf[...] = x_ref[...].astype(jnp.bfloat16)
        pl.semaphore_wait(barrier, 1)

        rdma = pltpu.make_async_remote_copy(
            src_ref=send_buf,
            dst_ref=recv_buf,
            send_sem=send_sem,
            recv_sem=recv_sem,
            device_id=peer,
            device_id_type=pl.DeviceIdType.MESH,
        )
        rdma.start()
        rdma.wait_recv()
        o_ref[...] = x_ref[...] + recv_buf[...].astype(jnp.float32)
        rdma.wait_send()

    return pl.pallas_call(
        kernel_body,
        out_shape=jax.ShapeDtypeStruct(x.shape, x.dtype),
        in_specs=[pl.BlockSpec(memory_space=pltpu.VMEM)],
        out_specs=pl.BlockSpec(memory_space=pltpu.VMEM),
        scratch_shapes=[
            pltpu.VMEM(x.shape, jnp.bfloat16),
            pltpu.VMEM(x.shape, jnp.bfloat16),
            pltpu.SemaphoreType.DMA,
            pltpu.SemaphoreType.DMA,
        ],
        compiler_params=pltpu.CompilerParams(collective_id=0),
    )(x)
```

```python
import jax
import jax.numpy as jnp
from jax import lax
from jax.experimental import pallas as pl
from jax.experimental.pallas import tpu as pltpu

BANDS = 32
TILES = 2 * BANDS
LINES = 8 * TILES

RAW_0 = 3
RAW_1 = 2
RELAY_START = 8 * RAW_1
RELAY_END = 100
DIRECT_END = 8 * (TILES - RAW_0)
RELAY_LINES = 4
RELAY_RAW_ROWS = 4
RELAY_PIECES = RELAY_START // RELAY_RAW_ROWS + (RELAY_END - RELAY_START) // RELAY_LINES
RELAY_LAST_BAND = (RELAY_END - 1) // 16

LOADS_0 = (6, 7, 8, 9, 11, 15, 31)
SENDS_0 = (6, 7, 8, 9, 11, 15, 26, 30, 31)
LOADS_1 = (1, 2, 3, 4, 5, 7, 11, 32)
SENDS_1 = (6, 7, 11, 27, 31, 32)
EARLY_LOADS_0 = 2
EARLY_LOADS_1 = 3


def _spans(bounds):
    return list(zip(bounds[:-1], bounds[1:]))


def _rows(first_band, end_band):
    return pl.ds(8 * first_band, 8 * (end_band - first_band))


def _lines(first, end):
    return pl.ds(first, end - first)


def _tile(t, row=0, rows=8):
    return pl.ds(8 * (t // 2) + row, rows), pl.ds(128 * (t % 2), 128)


def _all_reduce_y(
    x_hbm, out_ref, x_ref, send_buf, recv_buf, raw_buf,
    load_sems, send_sems, recv_sems,
    piece_send_sems, piece_recv_sems, relay_send_sems, relay_recv_sems,
):
    my_x = lax.axis_index("x")
    my_y = lax.axis_index("y")
    y_peer = (my_x, 1 - my_y)
    x_peer = (1 - my_x, my_y)
    barrier = pltpu.get_barrier_semaphore()

    def signal_entry(device):
        pl.semaphore_signal(
            barrier, inc=1, device_id=device, device_id_type=pl.DeviceIdType.MESH
        )

    def remote_copy(src, dst, send_sem, recv_sem, device):
        return pltpu.make_async_remote_copy(
            src_ref=src,
            dst_ref=dst,
            send_sem=send_sem,
            recv_sem=recv_sem,
            device_id=device,
            device_id_type=pl.DeviceIdType.MESH,
        )

    def wait_filled(region, recv_sem):
        pltpu.make_async_copy(region, region, recv_sem).wait()

    def make_loads(spans):
        return [
            pltpu.make_async_copy(x_hbm.at[_rows(*s)], x_ref.at[_rows(*s)], load_sems.at[i])
            for i, s in enumerate(spans)
        ]

    def start_all(copies):
        for copy in copies:
            copy.start()

    def wait_sent(copies):
        for copy in copies:
            copy.wait_send()

    def pack_and_send(spans, loads, sends):
        for (first, end), load in zip(spans, loads):
            load.wait()
            for b in range(first, end):
                v = x_ref[_rows(b, b + 1), :]
                both = jnp.concatenate([v[:, :128], v[:, 128:]], axis=0)
                send_buf[_lines(16 * b, 16 * b + 16), :] = both.astype(jnp.bfloat16)
            start_all(copy for end_line, copy in sends if 16 * first < end_line <= 16 * end)

    def add(first, end, raw_slot):
        for b in range(first, end):
            if 2 * b not in raw_slot and 2 * b + 1 not in raw_slot:
                r = recv_buf[_lines(16 * b, 16 * b + 16), :].astype(jnp.float32)
                r = jnp.concatenate([r[:8], r[8:]], axis=1)
                out_ref[_rows(b, b + 1), :] = x_ref[_rows(b, b + 1), :] + r
                continue
            for t in (2 * b, 2 * b + 1):
                if t in raw_slot:
                    r = raw_buf[pl.ds(8 * raw_slot[t], 8), :]
                else:
                    r = recv_buf[_lines(8 * t, 8 * t + 8), :].astype(jnp.float32)
                out_ref[_tile(t)] = x_ref[_tile(t)] + r

    relay_split = 16 * RELAY_LAST_BAND

    @pl.when(my_x == 0)
    def _():
        raw_slot = {t: t for t in range(RAW_1)}
        raw_slot.update({TILES - RAW_0 + k: RAW_1 + k for k in range(RAW_0)})
        spans = _spans(LOADS_0)
        loads = make_loads(spans + [(0, LOADS_0[0]), (LOADS_0[-1], BANDS)])
        start_all(loads[:EARLY_LOADS_0])
        pl.when(my_y == 0)(lambda: start_all(loads[EARLY_LOADS_0:]))

        signal_entry(y_peer)
        signal_entry(x_peer)
        pl.semaphore_wait(barrier, 1)

        raw_sends = [
            remote_copy(
                x_hbm.at[_tile(TILES - RAW_0 + k)], raw_buf.at[pl.ds(8 * (RAW_1 + k), 8)],
                piece_send_sems.at[k], piece_recv_sems.at[0], y_peer,
            )
            for k in range(RAW_0)
        ]
        start_all(raw_sends)
        pl.when(my_y == 1)(lambda: start_all(loads[EARLY_LOADS_0:]))

        sends = []
        for k, (first, end) in enumerate(_spans(SENDS_0)):
            end_line = min(16 * end, DIRECT_END)
            lines = _lines(max(16 * first, RELAY_END), end_line)
            copy = remote_copy(
                send_buf.at[lines], recv_buf.at[lines],
                send_sems.at[k], recv_sems.at[k], y_peer,
            )
            sends.append((end_line, copy))
        pack_and_send(spans, loads, sends)
        for load in loads[len(spans):]:
            load.wait()

        wait_filled(raw_buf.at[pl.ds(8 * RAW_1, 8 * RAW_0)], piece_recv_sems.at[0])
        add(SENDS_0[-1], BANDS, raw_slot)
        for (first, end), (_, copy) in zip(_spans(SENDS_0), sends):
            if end == SENDS_0[-2]:
                wait_sent(raw_sends + [c for _, c in sends])
            if end == SENDS_0[-1]:
                wait_filled(raw_buf.at[pl.ds(0, 8 * RAW_1)], relay_recv_sems.at[0])
                wait_filled(recv_buf.at[_lines(RELAY_START, relay_split)], relay_recv_sems.at[1])
                add(0, RELAY_LAST_BAND, raw_slot)
                wait_filled(recv_buf.at[_lines(relay_split, RELAY_END)], relay_recv_sems.at[2])
                add(RELAY_LAST_BAND, RELAY_LAST_BAND + 1, raw_slot)
            copy.wait_recv()
            add(max(first, RELAY_LAST_BAND + 1), end, raw_slot)

    @pl.when(my_x == 1)
    def _():
        raw_slot = {t: t for t in range(RAW_1)}
        signal_entry(y_peer)
        spans = _spans(LOADS_1)
        loads = make_loads(spans + [(0, LOADS_1[0])])
        start_all(loads[:EARLY_LOADS_1])
        pl.when(my_y == 0)(lambda: start_all(loads[EARLY_LOADS_1:]))
        pl.semaphore_wait(barrier, 2)

        pieces = []
        relays = []

        def add_piece(src, dst, relay_recv_sem):
            k = len(pieces)
            pieces.append(
                remote_copy(src, dst, piece_send_sems.at[k], piece_recv_sems.at[k], y_peer)
            )
            relays.append(remote_copy(dst, dst, relay_send_sems.at[k], relay_recv_sem, x_peer))
            return pieces[-1]

        for t in range(RAW_1):
            for row in range(0, 8, RELAY_RAW_ROWS):
                add_piece(
                    x_hbm.at[_tile(t, row, RELAY_RAW_ROWS)],
                    raw_buf.at[pl.ds(8 * t + row, RELAY_RAW_ROWS)],
                    relay_recv_sems.at[0],
                ).start()
        pl.when(my_y == 1)(lambda: start_all(loads[EARLY_LOADS_1:]))

        sends = []
        for line in range(RELAY_START, RELAY_END, RELAY_LINES):
            lines = pl.ds(line, RELAY_LINES)
            copy = add_piece(
                send_buf.at[lines], recv_buf.at[lines],
                relay_recv_sems.at[1 if line < relay_split else 2],
            )
            sends.append((line + RELAY_LINES, copy))
        rest = []
        for k, (first, end) in enumerate(_spans(SENDS_1)):
            lines = _lines(max(16 * first, RELAY_END), 16 * end)
            copy = remote_copy(
                send_buf.at[lines], recv_buf.at[lines],
                send_sems.at[k], recv_sems.at[k], y_peer,
            )
            rest.append(copy)
            sends.append((16 * end, copy))
        pack_and_send(spans, loads, sends)
        loads[-1].wait()

        for piece, relay in zip(pieces, relays):
            piece.wait_recv()
            relay.start()

        add(0, SENDS_1[0], raw_slot)
        wait_sent(pieces + relays)
        for (first, end), copy in zip(_spans(SENDS_1), rest):
            if end == BANDS:
                wait_sent(rest)
            copy.wait_recv()
            add(first, end, raw_slot)


def pallas_dist_ar_xy_y_m256_n256_kernel(x: jax.Array):
    assert x.shape == (8 * BANDS, 256) and x.dtype == jnp.float32
    n_sends = max(len(SENDS_0), len(SENDS_1)) - 1
    return pl.pallas_call(
        _all_reduce_y,
        out_shape=jax.ShapeDtypeStruct(x.shape, x.dtype),
        in_specs=[pl.BlockSpec(memory_space=pltpu.HBM)],
        out_specs=pl.BlockSpec(memory_space=pltpu.VMEM),
        scratch_shapes=[
            pltpu.VMEM(x.shape, jnp.float32),
            pltpu.VMEM((LINES, 128), jnp.bfloat16),
            pltpu.VMEM((LINES, 128), jnp.bfloat16),
            pltpu.VMEM((8 * (RAW_1 + RAW_0), 128), jnp.float32),
            pltpu.SemaphoreType.DMA((max(len(LOADS_0) + 1, len(LOADS_1)),)),
            pltpu.SemaphoreType.DMA((n_sends,)),
            pltpu.SemaphoreType.DMA((n_sends,)),
            pltpu.SemaphoreType.DMA((RELAY_PIECES,)),
            pltpu.SemaphoreType.DMA((RELAY_PIECES,)),
            pltpu.SemaphoreType.DMA((RELAY_PIECES,)),
            pltpu.SemaphoreType.DMA((3,)),
        ],
        compiler_params=pltpu.CompilerParams(
            collective_id=0,
            disable_bounds_checks=True,
            disable_semaphore_checks=True,
        ),
    )(x)
```

```python
import jax
import jax.numpy as jnp
from jax import lax
from jax.experimental import pallas as pl
from jax.experimental.pallas import tpu as pltpu

BANDS = 32
TILES = 2 * BANDS
LINES = 8 * TILES

RAW_0 = 3
RAW_1 = 2
RELAY_START = 8 * RAW_1
RELAY_END = 102
DIRECT_END = 8 * (TILES - RAW_0)
RELAY_LINES = 2
RELAY_RAW_ROWS = 2
RELAY_PIECES = RELAY_START // RELAY_RAW_ROWS + (RELAY_END - RELAY_START) // RELAY_LINES
RELAY_LAST_BAND = (RELAY_END - 1) // 16

LOADS_0 = (6, 7, 8, 9, 11, 15, 31)
SENDS_0 = (6, 7, 8, 9, 11, 15, 26, 30, 31)
LOADS_1 = (1, 2, 3, 4, 5, 7, 11, 32)
SENDS_1 = (6, 7, 11, 27, 31, 32)
EARLY_LOADS_0 = 2
EARLY_LOADS_1 = 3


def _spans(bounds):
    return list(zip(bounds[:-1], bounds[1:]))


def _rows(first_band, end_band):
    return pl.ds(8 * first_band, 8 * (end_band - first_band))


def _lines(first, end):
    return pl.ds(first, end - first)


def _tile(t, row=0, rows=8):
    return pl.ds(8 * (t // 2) + row, rows), pl.ds(128 * (t % 2), 128)


def _all_reduce_y(
    x_hbm, out_ref, x_ref, send_buf, recv_buf, raw_buf,
    load_sems, send_sems, recv_sems,
    piece_send_sems, piece_recv_sems, relay_send_sems, relay_recv_sems,
):
    my_x = lax.axis_index("x")
    my_y = lax.axis_index("y")
    y_peer = (my_x, 1 - my_y)
    x_peer = (1 - my_x, my_y)
    barrier = pltpu.get_barrier_semaphore()

    def signal_entry(device):
        pl.semaphore_signal(
            barrier, inc=1, device_id=device, device_id_type=pl.DeviceIdType.MESH
        )

    def remote_copy(src, dst, send_sem, recv_sem, device):
        return pltpu.make_async_remote_copy(
            src_ref=src,
            dst_ref=dst,
            send_sem=send_sem,
            recv_sem=recv_sem,
            device_id=device,
            device_id_type=pl.DeviceIdType.MESH,
        )

    def wait_filled(region, recv_sem):
        pltpu.make_async_copy(region, region, recv_sem).wait()

    def make_loads(spans):
        return [
            pltpu.make_async_copy(x_hbm.at[_rows(*s)], x_ref.at[_rows(*s)], load_sems.at[i])
            for i, s in enumerate(spans)
        ]

    def start_all(copies):
        for copy in copies:
            copy.start()

    def wait_sent(copies):
        for copy in copies:
            copy.wait_send()

    def pack_and_send(spans, loads, sends):
        for (first, end), load in zip(spans, loads):
            load.wait()
            for b in range(first, end):
                v = x_ref[_rows(b, b + 1), :]
                both = jnp.concatenate([v[:, :128], v[:, 128:]], axis=0)
                send_buf[_lines(16 * b, 16 * b + 16), :] = both.astype(jnp.bfloat16)
            start_all(copy for end_line, copy in sends if 16 * first < end_line <= 16 * end)

    def add(first, end, raw_slot):
        for b in range(first, end):
            if 2 * b not in raw_slot and 2 * b + 1 not in raw_slot:
                r = recv_buf[_lines(16 * b, 16 * b + 16), :].astype(jnp.float32)
                r = jnp.concatenate([r[:8], r[8:]], axis=1)
                out_ref[_rows(b, b + 1), :] = x_ref[_rows(b, b + 1), :] + r
                continue
            for t in (2 * b, 2 * b + 1):
                if t in raw_slot:
                    r = raw_buf[pl.ds(8 * raw_slot[t], 8), :]
                else:
                    r = recv_buf[_lines(8 * t, 8 * t + 8), :].astype(jnp.float32)
                out_ref[_tile(t)] = x_ref[_tile(t)] + r

    relay_split = 16 * RELAY_LAST_BAND

    @pl.when(my_x == 0)
    def _():
        raw_slot = {t: t for t in range(RAW_1)}
        raw_slot.update({TILES - RAW_0 + k: RAW_1 + k for k in range(RAW_0)})
        signal_entry(x_peer)
        spans = _spans(LOADS_0)
        loads = make_loads(spans + [(0, LOADS_0[0]), (LOADS_0[-1], BANDS)])
        start_all(loads[:EARLY_LOADS_0])
        signal_entry(y_peer)
        pl.semaphore_wait(barrier, 1)

        raw_sends = [
            remote_copy(
                x_hbm.at[_tile(TILES - RAW_0 + k)], raw_buf.at[pl.ds(8 * (RAW_1 + k), 8)],
                piece_send_sems.at[k], piece_recv_sems.at[0], y_peer,
            )
            for k in range(RAW_0)
        ]
        start_all(raw_sends)
        start_all(loads[EARLY_LOADS_0:])

        sends = []
        for k, (first, end) in enumerate(_spans(SENDS_0)):
            end_line = min(16 * end, DIRECT_END)
            lines = _lines(max(16 * first, RELAY_END), end_line)
            copy = remote_copy(
                send_buf.at[lines], recv_buf.at[lines],
                send_sems.at[k], recv_sems.at[k], y_peer,
            )
            sends.append((end_line, copy))
        pack_and_send(spans, loads, sends)
        for load in loads[len(spans):]:
            load.wait()

        wait_filled(raw_buf.at[pl.ds(8 * RAW_1, 8 * RAW_0)], piece_recv_sems.at[0])
        add(SENDS_0[-1], BANDS, raw_slot)
        for (first, end), (_, copy) in zip(_spans(SENDS_0), sends):
            if end == SENDS_0[-2]:
                wait_sent(raw_sends + [c for _, c in sends])
            if end == SENDS_0[-1]:
                wait_filled(raw_buf.at[pl.ds(0, 8 * RAW_1)], relay_recv_sems.at[0])
                wait_filled(recv_buf.at[_lines(RELAY_START, relay_split)], relay_recv_sems.at[1])
                add(0, RELAY_LAST_BAND, raw_slot)
                wait_filled(recv_buf.at[_lines(relay_split, RELAY_END)], relay_recv_sems.at[2])
                add(RELAY_LAST_BAND, RELAY_LAST_BAND + 1, raw_slot)
            copy.wait_recv()
            add(max(first, RELAY_LAST_BAND + 1), end, raw_slot)

    @pl.when(my_x == 1)
    def _():
        raw_slot = {t: t for t in range(RAW_1)}
        signal_entry(y_peer)
        spans = _spans(LOADS_1)
        loads = make_loads(spans + [(0, LOADS_1[0])])
        start_all(loads[:EARLY_LOADS_1])
        pl.when(my_y == 0)(lambda: start_all(loads[EARLY_LOADS_1:]))
        pl.semaphore_wait(barrier, 2)

        pieces = []
        relays = []

        def add_piece(src, dst, relay_recv_sem):
            k = len(pieces)
            pieces.append(
                remote_copy(src, dst, piece_send_sems.at[k], piece_recv_sems.at[k], y_peer)
            )
            relays.append(remote_copy(dst, dst, relay_send_sems.at[k], relay_recv_sem, x_peer))
            return pieces[-1]

        for t in range(RAW_1):
            for row in range(0, 8, RELAY_RAW_ROWS):
                add_piece(
                    x_hbm.at[_tile(t, row, RELAY_RAW_ROWS)],
                    raw_buf.at[pl.ds(8 * t + row, RELAY_RAW_ROWS)],
                    relay_recv_sems.at[0],
                ).start()
        pl.when(my_y == 1)(lambda: start_all(loads[EARLY_LOADS_1:]))

        sends = []
        for line in range(RELAY_START, RELAY_END, RELAY_LINES):
            lines = pl.ds(line, RELAY_LINES)
            copy = add_piece(
                send_buf.at[lines], recv_buf.at[lines],
                relay_recv_sems.at[1 if line < relay_split else 2],
            )
            sends.append((line + RELAY_LINES, copy))
        rest = []
        for k, (first, end) in enumerate(_spans(SENDS_1)):
            lines = _lines(max(16 * first, RELAY_END), 16 * end)
            copy = remote_copy(
                send_buf.at[lines], recv_buf.at[lines],
                send_sems.at[k], recv_sems.at[k], y_peer,
            )
            rest.append(copy)
            sends.append((16 * end, copy))
        pack_and_send(spans, loads, sends)
        loads[-1].wait()

        for piece, relay in zip(pieces, relays):
            piece.wait_recv()
            relay.start()

        add(0, SENDS_1[0], raw_slot)
        wait_sent(pieces + relays)
        for (first, end), copy in zip(_spans(SENDS_1), rest):
            if end == BANDS:
                wait_sent(rest)
            copy.wait_recv()
            add(first, end, raw_slot)


def pallas_dist_ar_xy_y_m256_n256_kernel(x: jax.Array):
    assert x.shape == (8 * BANDS, 256) and x.dtype == jnp.float32
    n_sends = max(len(SENDS_0), len(SENDS_1)) - 1
    return pl.pallas_call(
        _all_reduce_y,
        out_shape=jax.ShapeDtypeStruct(x.shape, x.dtype),
        in_specs=[pl.BlockSpec(memory_space=pl.ANY)],
        out_specs=pl.BlockSpec(memory_space=pltpu.VMEM),
        scratch_shapes=[
            pltpu.VMEM(x.shape, jnp.float32),
            pltpu.VMEM((LINES, 128), jnp.bfloat16),
            pltpu.VMEM((LINES, 128), jnp.bfloat16),
            pltpu.VMEM((8 * (RAW_1 + RAW_0), 128), jnp.float32),
            pltpu.SemaphoreType.DMA((max(len(LOADS_0) + 1, len(LOADS_1)),)),
            pltpu.SemaphoreType.DMA((n_sends,)),
            pltpu.SemaphoreType.DMA((n_sends,)),
            pltpu.SemaphoreType.DMA((RELAY_PIECES,)),
            pltpu.SemaphoreType.DMA((RELAY_PIECES,)),
            pltpu.SemaphoreType.DMA((RELAY_PIECES,)),
            pltpu.SemaphoreType.DMA((3,)),
        ],
        compiler_params=pltpu.CompilerParams(
            collective_id=0,
            disable_bounds_checks=True,
            disable_semaphore_checks=True,
        ),
    )(x)
```
